```python
import numpy as np

kernel_name = "dist_rs_xy_x_m65536_n1024"

def setup_inputs():
    return {"x": np.random.randn(2, 65536, 1024).astype(np.float32)}

def reference(x: np.ndarray) -> np.ndarray:
    return x.sum(axis=0)
```

```python
import jax
import jax.numpy as jnp
from jax import lax
from jax.experimental import pallas as pl
from jax.experimental.pallas import tpu as pltpu

MESH = pl.DeviceIdType.MESH


def make_kernel(R=256, D=2, NB=6, out_f32=False, vmem=32):
    def kernel(x):
        _, m, n = x.shape
        w = n // 2
        h = m // 2
        nch = h // R
        NS = D + 1

        def body(x_ref, o_ref, fin, sbuf, fin_sem, sx_sem, sy_sem, rx_sem, ry_sem):
            mx = lax.axis_index("x")
            my = lax.axis_index("y")
            xn = (1 - mx, my)
            yn = (mx, 1 - my)
            mine = pl.ds(pl.multiple_of(mx * w, w), w)
            theirs = pl.ds(pl.multiple_of((1 - mx) * w, w), w)
            row_a = my * h
            row_b = (1 - my) * h

            def rows(base, i):
                return pl.ds(pl.multiple_of(base + i * R, R), R)

            def load(i):
                return pltpu.make_async_copy(x_ref.at[0, rows(row_a, i)], fin.at[i % NB], fin_sem.at[i % NB])

            def send_x(i):
                return pltpu.make_async_remote_copy(
                    sbuf.at[i % NS], o_ref.at[rows(row_a, i)], sx_sem.at[i % NS], rx_sem.at[i],
                    device_id=xn, device_id_type=MESH)

            def send_y(i):
                return pltpu.make_async_remote_copy(
                    o_ref.at[rows(row_a, i)], o_ref.at[rows(row_a, i)], sy_sem, ry_sem,
                    device_id=yn, device_id_type=MESH)

            barrier = pltpu.get_barrier_semaphore()
            pl.semaphore_signal(barrier, 1, device_id=xn, device_id_type=MESH)
            pl.semaphore_signal(barrier, 1, device_id=yn, device_id_type=MESH)
            for i in range(NB):
                load(i).start()

            def produce(i):
                load(i).wait()
                sbuf[i % NS] = fin[i % NB, :, theirs].astype(jnp.bfloat16)

            produce(0)
            pl.semaphore_wait(barrier, 2)
            send_x(0).start()
            for i in range(1, D):
                produce(i)
                send_x(i).start()

            def step(i, c):
                send_x(i).wait_recv()
                r = rows(row_a, i)
                o_ref[r, :] = (fin[i % NB, :, mine] + o_ref[r, :].astype(jnp.float32)).astype(jnp.bfloat16)
                send_y(i).start()

                @pl.when(i + NB < nch)
                def _():
                    load(i + NB).start()

                j = i + D

                @pl.when(j < nch)
                def _():
                    @pl.when(j >= NS)
                    def _():
                        send_x(j - NS).wait_send()

                    produce(j)
                    send_x(j).start()

                return c

            lax.fori_loop(0, nch, step, 0)
            for i in range(nch - NS, nch):
                send_x(i).wait_send()
            half_a = o_ref.at[pl.ds(pl.multiple_of(row_a, h), h)]
            half_b = o_ref.at[pl.ds(pl.multiple_of(row_b, h), h)]
            pltpu.make_async_copy(half_a, half_a, sy_sem).wait()
            pltpu.make_async_copy(half_b, half_b, ry_sem).wait()

        dma = pltpu.SemaphoreType.DMA
        out = pl.pallas_call(
            body,
            out_shape=pltpu.VMEM((m, w), jnp.bfloat16),
            in_specs=[pl.BlockSpec(memory_space=pl.ANY)],
            out_specs=pl.BlockSpec(memory_space=pltpu.VMEM),
            scratch_shapes=[
                pltpu.VMEM((NB, R, n), jnp.float32),
                pltpu.VMEM((NS, R, w), jnp.bfloat16),
                dma((NB,)), dma((NS,)), dma, dma((nch,)), dma,
            ],
            compiler_params=pltpu.CompilerParams(collective_id=0, vmem_limit_bytes=vmem * 2**20),
        )(x)
        return out.astype(jnp.float32) if out_f32 else out

    return kernel


pallas_dist_rs_xy_x_m65536_n1024_kernel = make_kernel(R=128)
```

```python
import jax
import jax.numpy as jnp
import numpy as np
from jax import lax
from jax.experimental import pallas as pl
from jax.experimental.pallas import tpu as pltpu

MESH = pl.DeviceIdType.MESH
ONES = 0x01010101
HDR_BITS = 20
TILE = (8, 128)
BLK = 64


def _c(v):
    return np.uint32(v).astype(np.int32)


def shr(a, b):
    if not isinstance(b, jax.Array):
        b = jnp.full(a.shape, b, jnp.int32)
    return lax.shift_right_logical(a, b)


def ge(x, k):
    return shr(x + _c((0x80 - k) * ONES), 7) & _c(ONES)


def tile(a, j):
    return a[(j // 4) * 8:(j // 4 + 1) * 8, (j % 4) * 128:(j % 4 + 1) * 128]


def gather(f):
    return jnp.concatenate([jnp.concatenate([f(4 * r + c) for c in range(4)], axis=1) for r in range(2)], axis=0)


def first_lane():
    return (lax.broadcasted_iota(jnp.int32, TILE, 0) | lax.broadcasted_iota(jnp.int32, TILE, 1)) == 0


def lookup(table, k):
    out = jnp.int32(table[0])
    for i in range(1, len(table)):
        if table[i] != table[i - 1]:
            out = jnp.where(k >= i, table[i], out)
    return out


def make_kernel(NBLK=32, P=8, LEAD=4, nc=16, back=12, K=3, E=3, LY=2, NF=4, enc=(1, 3, 5, 8), dec=(2, 4, 6, 7, 8),
                out_f32=False, vmem=48, dbg=""):
    BPP = NBLK // P
    PR = BPP * BLK
    R = NBLK * BLK
    sign0 = 8 * NBLK
    w0 = sign0 + NBLK
    raw_words = 7 * NBLK + 1
    guard = nc - back + 3
    msg_words = w0 + raw_words + guard
    NP = P + 3
    kW, kD, kS = LEAD, LEAD + 1, LEAD + 2
    assert len(enc) == LEAD and enc[-1] == P and all(enc[i] > i for i in range(LEAD))
    enc_hi = list(enc) + [P] * (NP - LEAD)
    enc_lo = [0] + enc_hi[:-1]
    assert len(dec) == NP - kS and dec[-1] == P and all(dec[i] <= LEAD + i for i in range(len(dec)))
    dec_hi = [0] * kS + list(dec)
    dec_lo = [0] + dec_hi[:-1]

    def raw_slot(b, j):
        return sign0 + b if j == 0 else w0 + 7 * b + j

    def base_of(b, words):
        return ((b * words) >> (NBLK.bit_length() - 1)) - back

    def enc_begin(src, st):
        sample = jnp.abs(src[pl.ds(0, BLK), :])
        mean = jnp.sum(jnp.sum(sample, axis=0, keepdims=True), axis=1, keepdims=True) * (1.843 / sample.size)
        eb = shr(pltpu.bitcast(jnp.broadcast_to(mean, TILE), jnp.int32), 23) & 0xFF
        align = (eb + 1) & 1
        top = (shr(eb + align, 1) + 2) & 0x7F
        st[0] = jnp.where(first_lane(), HDR_BITS, 0)
        st[1] = jnp.zeros(TILE, jnp.int32)
        st[2] = jnp.zeros(TILE, jnp.int32)
        st[3] = (align << 7) | top

    def enc_part(src, p, msg, hi_ref, code_ref, st):
        key = st[3]
        bias = key & 0x80
        bias = jnp.tile(bias | (bias << 16), (2, 4))
        t4 = key | 0x80
        t4 = t4 | (t4 << 8)
        t4 = jnp.tile(t4 | (t4 << 16), (2, 4))

        def block(i, carry):
            total, any_x, any_n = carry
            b = p * BPP + i
            v = src[pl.ds(pl.multiple_of(i * BLK, BLK), BLK), :]
            w = pltpu.bitcast(v.astype(jnp.bfloat16), jnp.int32)
            wa = w[:16] + bias
            wb = w[16:] + bias
            t = (shr(wa, 8) ^ wb) & _c(0x00FF00FF)
            hi = wb ^ t
            lo = wa ^ (t << 8)
            x = (t4 - (hi & _c(0x7F7F7F7F))) & _c(0x7F7F7F7F)
            g1 = ge(x, 1)
            ln = x + _c(8 * ONES) + ge(x, 5) + ge(x, 8) - g1 - ((g1 + ge(x, 2)) << 2)
            e = ln + (ln << 8)
            e = e + (e << 16) - _c(ONES)
            top_bit = jnp.full(e.shape, _c(0x80000000), jnp.int32)
            code = shr(top_bit, e & 31)
            for k in (8, 16, 24):
                code = code | shr(top_bit, shr(e, k) & 31)
            n = shr(e, 24) + 1
            sign = hi & _c(0x80808080)
            for j in reversed(range(8)):
                msg[8 * b + j] = tile(lo, j)
                hi_ref[8 * b + j] = tile(hi, j)
                sj, nj, cj = tile(sign, j), tile(n, j), tile(code, j)
                any_x = any_x | tile(x, j)
                any_n = any_n | nj
                if j == 7:
                    s, bits, acc = shr(sj, j), nj, [cj]
                    continue
                s = s | (shr(sj, j) if j else sj)
                bits = bits + nj
                right = nj & 31
                left = (-nj) & 31
                new = [cj | shr(acc[0], right)]
                for k in range(1, min(len(acc) + 1, 3)):
                    u = acc[k - 1] << left
                    new.append(u | shr(acc[k], right) if k < len(acc) else u)
                acc = new
            msg[sign0 + b] = s
            for k in range(3):
                code_ref[4 * b + k] = acc[k]
            code_ref[4 * b + 3] = bits
            return total + bits, any_x | jnp.where(bits > 96, -1, 0), any_n

        st[0], st[1], st[2] = lax.fori_loop(0, BPP, block, (st[0], st[1], st[2]))

    def enc_finish(msg, hi_ref, code_ref, st):
        zero = jnp.zeros(TILE, jnp.int32)
        first = first_lane()
        bad = ((st[1] & _c(0x60606060)) | (st[2] & -32)) != 0
        words = jnp.max(jnp.where(bad, raw_words, jnp.minimum(shr(st[0] + 31, 5), raw_words)))

        def clear(j, c):
            msg[w0 + j] = zero
            return c

        lax.fori_loop(0, words + guard, clear, 0)

        def emit(b, carry):
            pos, drift = carry
            base = base_of(b, words)
            d = shr(pos, 5) - base
            s = pos & 31
            r = 31 - s
            a = [code_ref[4 * b + k] for k in range(3)]
            up = [(v << 1) << r for v in a]
            dn = [shr(v, s) for v in a]
            v = [dn[0], dn[1] | up[0], dn[2] | up[1], up[2]]
            step = 1
            while step < nc:
                m = (d & step) != 0
                v = [jnp.where(m, v[k - step] if 0 <= k - step < len(v) else zero, v[k] if k < len(v) else zero)
                     for k in range(min(len(v) + step, nc + 3))]
                step *= 2
            at = w0 + base
            for k in range(len(v)):
                msg[at + k] = msg[at + k] | v[k]
            return pos + code_ref[4 * b + 3], drift | d | (nc - 1 - d)

        blocks = jnp.where(words < raw_words, NBLK, 0)
        _, drift = lax.fori_loop(0, blocks, emit, (jnp.where(first, HDR_BITS, 0), zero))
        words = jnp.max(jnp.where(drift < 0, raw_words, words))

        @pl.when(words == raw_words)
        def _():
            msg[w0] = zero

            def raw(b, c):
                for j in range(8):
                    msg[raw_slot(b, j)] = hi_ref[8 * b + j]
                return c

            lax.fori_loop(0, NBLK, raw, 0)

        msg[w0] = msg[w0] | jnp.where(first, (st[3] | (words << 8)) << (32 - HDR_BITS), 0)
        return words

    def dec_part(msg, hdr, p, pos_ref, write):
        wide = (16, 512)
        words = hdr >> 8
        bias = jnp.full(wide, ((hdr >> 7) & 1) * 0x00800080, jnp.int32)
        t4 = jnp.full(wide, ((hdr & 0x7F) | 0x80) * ONES, jnp.int32)

        def finish(i, hi):
            b = p * BPP + i
            lo = gather(lambda j: msg[8 * b + j])
            t = (shr(lo, 8) ^ hi) & _c(0x00FF00FF)
            wa = (lo ^ (t << 8)) - bias
            wb = (hi ^ t) - bias
            write(pl.multiple_of(i * BLK, BLK), pltpu.bitcast(jnp.concatenate([wa, wb], axis=0), jnp.bfloat16))

        @pl.when(words == raw_words)
        def _():
            def raw(i, c):
                finish(i, gather(lambda j: msg[raw_slot(p * BPP + i, j)]))
                return c

            lax.fori_loop(0, BPP, raw, 0)

        @pl.when(words < raw_words)
        def _():
            def coded(i, pos):
                b = p * BPP + i
                base = base_of(b, words)
                d = shr(pos, 5) - base
                c = [msg[w0 + base + k] for k in range(nc + 3)]
                step = pl.next_power_of_2(nc) // 2
                while step:
                    m = (d & step) != 0
                    c = [jnp.where(m, c[k + step], c[k]) if k + step < len(c) else c[k] for k in range(step + 3)]
                    step //= 2
                s = pos & 31
                r = 31 - s
                win = [(c[k] << s) | shr(shr(c[k + 1], 1), r) for k in range(3)]
                ranks = []
                for j in range(8):
                    u = win[0]
                    for k in range(4):
                        z = lax.clz(u)
                        if k < 3:
                            u = (u << 1) << z
                        n = z + 4 if k == 0 else n + z
                        r = z if k == 0 else r | (z << (8 * k))
                    ranks.append(r)
                    pos = pos + n
                    left = 32 - n
                    win = [(win[k] << n) | shr(win[k + 1], left) if k + 1 < len(win) else win[k] << n
                           for k in range(min(3, 7 - j))]
                r = gather(lambda j: ranks[j])
                g8 = ge(r, 8)
                g4 = ge(r, 4)
                x = r + _c(2 * ONES) + ((g4 + (g8 << 1)) << 2) - g4 - g8 - ((ge(r, 3) + (ge(r, 7) << 1)) << 2)
                sg = msg[sign0 + b]
                sign = gather(lambda j: sg << j if j else sg) & _c(0x80808080)
                finish(i, ((t4 - x) & _c(0x7F7F7F7F)) | sign)
                return pos

            pos_ref[...] = lax.fori_loop(0, BPP, coded, pos_ref[...])

    def kernel(x):
        _, m, n = x.shape
        w = n // 2
        h = m // 2
        nch = h // R
        nparts = nch * P
        assert w == 512 and h % R == 0 and nch > K

        def body(x_ref, o_ref, fe, fx, fy, tx, rx, ry, hi_ref, code_ref, st, pos, hdrs,
                 fe_sem, fx_sem, fy_sem, tx_sem, fw_sem, rx_sem, ry_sem, cx_sem, cy_sem):
            mx = lax.axis_index("x")
            my = lax.axis_index("y")
            xn = (1 - mx, my)
            yn = (mx, 1 - my)
            mine = pl.ds(pl.multiple_of(mx * w, w), w)
            theirs = pl.ds(pl.multiple_of((1 - mx) * w, w), w)
            row_a = my * h
            row_b = (1 - my) * h

            def loader(row0, cols, buf, sem):
                def make(g):
                    rows = pl.ds(pl.multiple_of(row0 + g * PR, PR), PR)
                    return pltpu.make_async_copy(x_ref.at[0, rows, cols], buf.at[g % NF], sem.at[g % NF])
                return make

            load_e = loader(row_a, theirs, fe, fe_sem)
            load_x = loader(row_a, mine, fx, fx_sem)
            load_y = loader(row_b, mine, fy, fy_sem)

            def piece(src, dst, send_sem, recv_sem, dev, slot, k, words, act):
                def go(span):
                    act(pltpu.make_async_remote_copy(
                        src.at[slot, span], dst.at[slot, span], send_sem.at[slot], recv_sem.at[slot * NP + k],
                        device_id=dev, device_id_type=MESH))

                @pl.when((k < kW) | (k > kS))
                def _():
                    go(pl.ds(jnp.where(k < kW, k, k - 3) * (8 * BPP), 8 * BPP))

                @pl.when((k == kW) | (k == kS))
                def _():
                    go(pl.ds(jnp.where(k == kW, w0, sign0), NBLK))

                @pl.when(k == kD)
                def _():
                    go(pl.ds(w0 + NBLK, words() - NBLK))

            def whole(buf, sem, slot, words):
                v = buf.at[slot, pl.ds(0, w0 + words)]
                return pltpu.make_async_copy(v, v, sem.at[slot])

            def produce(c, k, first=False):
                slot = c % K
                msg = tx.at[slot]

                @pl.when((k == 0) & (c >= K))
                def _():
                    whole(tx, tx_sem, slot, hdrs[slot]).wait()

                def part(p, carry):
                    g = c * P + p
                    load_e(g).wait()

                    @pl.when(p == 0)
                    def _():
                        enc_begin(fe.at[g % NF], st)

                    enc_part(fe.at[g % NF], p, msg, hi_ref, code_ref, st)

                    @pl.when(g + NF < nparts)
                    def _():
                        load_e(g + NF).start()

                    return carry

                lax.fori_loop(lookup(enc_lo, k), lookup(enc_hi, k), part, 0)

                @pl.when(k == kW)
                def _():
                    hdrs[slot] = enc_finish(msg, hi_ref, code_ref, st)

                @pl.when((k == 0) & (c == 0))
                def _():
                    pl.semaphore_wait(barrier, 2)

                @pl.when((k == 0) & (c >= K))
                def _():
                    pl.semaphore_wait(cx_sem.at[slot], 1)

                piece(tx, rx, tx_sem, rx_sem, xn, slot, k, lambda: hdrs[slot], lambda d: d.start())

            def arrive(buf, recv_sem, side, c, k):
                slot = c % K
                at = side * K + slot
                piece(buf, buf, fw_sem, recv_sem, yn, slot, k, lambda: hdrs[at] >> 8, lambda d: d.wait_recv())

                @pl.when(k == kW)
                def _():
                    hdrs[at] = shr(buf[slot, w0], 32 - HDR_BITS)[0, 0]

            def consume(buf, side, c, k, load, loc, row0):
                slot = c % K
                at = side * K + slot

                @pl.when(k == kS)
                def _():
                    pos[side - 1] = jnp.where(first_lane(), HDR_BITS, 0)
                    for j in range(guard):
                        buf[slot, w0 + (hdrs[at] >> 8) + j] = jnp.zeros(TILE, jnp.int32)

                def part(p, carry):
                    g = c * P + p
                    load(g).wait()

                    def write(r, v):
                        rows = pl.ds(pl.multiple_of(row0 + g * PR + r, BLK), BLK)
                        o_ref[rows, :] = (loc[g % NF, pl.ds(r, BLK), :] + v.astype(jnp.float32)).astype(jnp.bfloat16)

                    if "nodec" not in dbg:
                        dec_part(buf.at[slot], hdrs[at], p, pos.at[side - 1], write)

                    @pl.when(g + NF < nparts)
                    def _():
                        load(g + NF).start()

                    return carry

                lax.fori_loop(lookup(dec_lo, k), lookup(dec_hi, k), part, 0)

            barrier = pltpu.get_barrier_semaphore()
            for g in range(NF):
                load_e(g).start()
            pl.semaphore_signal(barrier, 1, device_id=xn, device_id_type=MESH)
            pl.semaphore_signal(barrier, 1, device_id=yn, device_id_type=MESH)

            def advance(c, k):
                wrap = k == NP - 1
                return jnp.where(wrap, c + 1, c), jnp.where(wrap, 0, k + 1)

            def step(t, carry):
                ce, ke, cx, kx, cy, ky = carry
                on_x = (cx >= 0) & (cx < nch)
                on_y = cy >= 0

                @pl.when(on_x)
                def _():
                    arrive(rx, rx_sem, 1, cx, kx)
                    slot = cx % K

                    @pl.when((kx == 0) & (cx >= K))
                    def _():
                        pl.semaphore_wait(cy_sem.at[slot], 1)

                    piece(rx, ry, fw_sem, ry_sem, yn, slot, kx, lambda: hdrs[K + slot] >> 8, lambda d: d.start())

                @pl.when(ce < nch)
                def _():
                    produce(ce, ke)

                @pl.when(t == E)
                def _():
                    for g in range(NF):
                        load_x(g).start()
                        load_y(g).start()

                @pl.when(on_x)
                def _():
                    consume(rx, 1, cx, kx, load_x, fx, row_a)

                    @pl.when((kx == 2) & (cx >= 1) & (cx - 1 + K < nch))
                    def _():
                        slot = (cx - 1) % K
                        whole(rx, fw_sem, slot, hdrs[K + slot] >> 8).wait()
                        pl.semaphore_signal(cx_sem.at[slot], 1, device_id=xn, device_id_type=MESH)

                @pl.when(on_y)
                def _():
                    arrive(ry, ry_sem, 2, cy, ky)
                    consume(ry, 2, cy, ky, load_y, fy, row_b)

                    @pl.when((ky == NP - 1) & (cy + K < nch))
                    def _():
                        pl.semaphore_signal(cy_sem.at[cy % K], 1, device_id=yn, device_id_type=MESH)

                return (*advance(ce, ke), *advance(cx, kx), *advance(cy, ky))

            i32 = jnp.int32
            init = (i32(0), i32(0), i32(-1), i32(NP - E), i32(-1), i32(NP - E - LY))
            lax.fori_loop(0, nch * NP + E + LY, step, init)
            for c in range(nch - K, nch):
                slot = c % K
                whole(tx, tx_sem, slot, hdrs[slot]).wait()
                whole(rx, fw_sem, slot, hdrs[K + slot] >> 8).wait()

        dma = pltpu.SemaphoreType.DMA
        reg = pltpu.SemaphoreType.REGULAR
        stage = pltpu.VMEM((NF, PR, w), jnp.float32)
        ring = pltpu.VMEM((K, msg_words, *TILE), jnp.int32)
        out = pl.pallas_call(
            body,
            out_shape=pltpu.VMEM((m, w), jnp.bfloat16),
            in_specs=[pl.BlockSpec(memory_space=pl.ANY)],
            out_specs=pl.BlockSpec(memory_space=pltpu.VMEM),
            scratch_shapes=[
                stage, stage, stage, ring, ring, ring,
                pltpu.VMEM((8 * NBLK, *TILE), jnp.int32),
                pltpu.VMEM((4 * NBLK, *TILE), jnp.int32),
                pltpu.VMEM((4, *TILE), jnp.int32),
                pltpu.VMEM((2, *TILE), jnp.int32),
                pltpu.SMEM((3 * K,), jnp.int32),
                dma((NF,)), dma((NF,)), dma((NF,)), dma((K,)), dma((K,)), dma((K * NP,)), dma((K * NP,)),
                reg((K,)), reg((K,)),
            ],
            compiler_params=pltpu.CompilerParams(collective_id=0, vmem_limit_bytes=vmem * 2**20),
        )(x)
        return out.astype(jnp.float32) if out_f32 else out

    return kernel


pallas_dist_rs_xy_x_m65536_n1024_kernel = make_kernel()
```

```python
import jax
import jax.numpy as jnp
import numpy as np
from jax import lax
from jax.experimental import pallas as pl
from jax.experimental.pallas import tpu as pltpu

MESH = pl.DeviceIdType.MESH

WORD = (8, 128)
COLS = 512
UNIT_ROWS = 128
BLOCK_WORDS = 9
UNIT_WORDS = 2 * BLOCK_WORDS
HEADER_BITS = 26
REFERENCE_OFFSET = 472


def _rep(byte):
    return np.uint32(byte * 0x01010101).astype(np.int32)


def _shr(a, n):
    if not isinstance(n, jax.Array):
        if n == 0:
            return a
        n = jnp.full(a.shape, n, jnp.int32)
    return lax.shift_right_logical(a, n)


def _log2(n):
    assert n & (n - 1) == 0
    return n.bit_length() - 1


def _swap_bytes(a, b):
    t = (_shr(a, 8) ^ b) & np.int32(0x00FF00FF)
    return a ^ (t << 8), b ^ t


def _to_rank(j):
    g4, g5, g9, g20 = ((j + _rep(0x80 - k)) & _rep(0x80) for k in (4, 5, 9, 20))
    return j + _rep(16) + _shr(g9, 7) + _shr(g20, 5) - _shr(g4, 3) - _shr(g5, 5) - _shr(g5, 7)


def _from_rank(r):
    a4, a5, a16, a20 = (r + _rep(0x80 - k) for k in (4, 5, 16, 20))
    is4 = (a4 ^ a5) & _rep(0x80)
    is_high = (a16 ^ a20) & _rep(0x80)
    return (r + _rep(5) - _shr(is4, 5) - _shr(a4 & _rep(0x80), 7)
            - _shr(is_high, 3) - _shr(a16 & _rep(0x80), 5))


def _in_first_lane(value):
    first = (lax.broadcasted_iota(jnp.int32, WORD, 0) | lax.broadcasted_iota(jnp.int32, WORD, 1)) == 0
    return jnp.where(first, value, 0)


class _Codec:
    def __init__(self, units, window, back, closing_steps):
        self.blocks = 2 * units
        self.window = window
        self.back = back
        self.closing_steps = closing_steps
        self.stream = UNIT_WORDS * units
        self.min_words = self.blocks
        self.raw_words = 7 * self.blocks + 1
        self.max_coded_words = self.raw_words - 8
        self.guard = window - back + 3
        self.message_words = self.stream + self.raw_words + self.guard
        assert self.raw_words < 1 << (HEADER_BITS - 16) and self.min_words >= back
        assert self.blocks % closing_steps == 0

    def scratch_shapes(self):
        return [
            pltpu.VMEM((8 * self.blocks, *WORD), jnp.int32),
            pltpu.VMEM((4 * self.blocks, *WORD), jnp.int32),
            pltpu.VMEM((3, *WORD), jnp.int32),
        ]

    def _base(self, b, words):
        return jnp.maximum(((b * words) >> _log2(self.blocks)) - self.back, 0)

    def open(self, src, scratch):
        state = scratch[2]
        sample = jnp.abs(src[pl.ds(0, 8)].reshape(64, COLS))
        total = jnp.sum(jnp.sum(sample, axis=0, keepdims=True), axis=1, keepdims=True)
        mean = jnp.broadcast_to(total * (1.0 / sample.size), WORD)
        state[0] = _in_first_lane(HEADER_BITS)
        state[1] = jnp.zeros(WORD, jnp.int32)
        state[2] = (_shr(pltpu.bitcast(mean, jnp.int32), 16) + REFERENCE_OFFSET) & 0xFFFF

    def encode_unit(self, src, u, msg, scratch):
        high_ref, code_ref, state = scratch
        total, misfit, reference = state[0], state[1], state[2]
        reference = jnp.tile(reference | (reference << 16), (8, 1))
        for i in range(2):
            b = 2 * u + i
            values = src[:, :, 256 * i:256 * (i + 1)].reshape(UNIT_ROWS, 256)
            pairs = pltpu.bitcast(values.astype(jnp.bfloat16), jnp.int32)
            low, high = _swap_bytes(reference - pairs[:, :128], reference - pairs[:, 128:])
            rank = _to_rank(((high & _rep(0x1F)) << 2) | (_shr(low, 6) & _rep(0x03)))
            low = (low & _rep(0x3F)) | ((rank << 6) & _rep(0xC0))
            group = _shr(rank, 2) & _rep(0x1F)
            sign = high & _rep(0x80)
            at = UNIT_WORDS * u + BLOCK_WORDS * i
            msg[pl.ds(at, 8)] = low.reshape(8, *WORD)
            high_ref[pl.ds(8 * b, 8)] = ((high & _rep(0x60)) | group).reshape(8, *WORD)

            stop = group + (group << 8)
            stop = stop + (stop << 16) + 0x03020100
            one = jnp.full(stop.shape, -2**31, jnp.int32)
            code = _shr(one, stop & 31)
            for shift in (8, 16, 24):
                code = code | _shr(one, _shr(stop, shift) & 31)
            length = _shr(stop, 24) + 1

            for j in reversed(range(8)):
                h, s, n, c = (a[8 * j:8 * j + 8] for a in (high, sign, length, code))
                if j == 7:
                    signs, bits, chain, any_high, any_length = _shr(s, j), n, [c], h, n
                    continue
                signs, bits = signs | _shr(s, j), bits + n
                any_high, any_length = any_high | h, any_length | n
                right, left = n & 31, (-n) & 31
                longer = [c | _shr(chain[0], right)]
                for k in range(1, min(len(chain) + 1, 3)):
                    carried = chain[k - 1] << left
                    longer.append(carried | _shr(chain[k], right) if k < len(chain) else carried)
                chain = longer
            msg[at + 8] = signs
            for k in range(3):
                code_ref[4 * b + k] = chain[k]
            code_ref[4 * b + 3] = bits
            total = total + bits
            misfit = misfit | (any_high & _rep(0x60)) | _shr(any_length, 5) | _shr(96 - bits, 31)
        state[0] = total
        state[1] = misfit

    def close(self, step, msg, scratch, words_ref, slot):
        high_ref, code_ref, state = scratch
        zero = jnp.zeros(WORD, jnp.int32)

        @pl.when(step == 0)
        def _():
            needed = jnp.maximum(_shr(state[0] + 31, 5), self.min_words)
            uncoded = (state[1] != 0) | (needed > self.max_coded_words)
            words = jnp.max(jnp.where(uncoded, self.raw_words, needed))
            words_ref[slot] = words
            state[0] = _in_first_lane(HEADER_BITS)

            @pl.loop(0, (jnp.minimum(words, self.max_coded_words) + self.guard + 7) >> 3)
            def _(j):
                msg[pl.ds(self.stream + 8 * j, 8)] = jnp.zeros((8, *WORD), jnp.int32)

        words = words_ref[slot]

        def append(b, carry):
            position, misfit = carry
            base = self._base(b, words)
            drift = _shr(position, 5) - base
            bit = position & 31
            rest = 31 - bit
            chain = [code_ref[4 * b + k] for k in range(3)]
            kept = [_shr(c, bit) for c in chain]
            carried = [(c << 1) << rest for c in chain]
            out = [kept[0], kept[1] | carried[0], kept[2] | carried[1], carried[2]]
            hop = 1
            while hop < self.window:
                moved = (drift & hop) != 0
                out = [
                    jnp.where(moved, out[k - hop] if 0 <= k - hop < len(out) else zero,
                              out[k] if k < len(out) else zero)
                    for k in range(min(len(out) + hop, self.window + 3))
                ]
                hop *= 2
            span = pl.ds(self.stream + base, self.window + 3)
            msg[span] = msg[span] | jnp.stack(out)
            outside = _shr(drift | (self.window - 1 - drift), 31)
            return position + code_ref[4 * b + 3], misfit | outside

        count = self.blocks // self.closing_steps
        first = step * count
        state[0], state[1] = lax.fori_loop(
            first, jnp.where(words < self.raw_words, first + count, first), append, (state[0], state[1]))

        @pl.when(step == self.closing_steps - 1)
        def _():
            final = jnp.max(jnp.where(state[1] != 0, self.raw_words, words))
            words_ref[slot] = final

            @pl.when(final == self.raw_words)
            def _():
                msg[self.stream] = zero

                @pl.loop(0, self.blocks)
                def _(b):
                    last = high_ref[8 * b + 7]
                    for j in range(7):
                        msg[self.stream + 1 + 7 * b + j] = (
                            high_ref[8 * b + j] | ((last << (j + 1)) & _rep(0x80)))

            header = ((final << 16) | state[2]) << (32 - HEADER_BITS)
            msg[self.stream] = msg[self.stream] | _in_first_lane(header)

    def header(self, msg):
        return _shr(msg[self.stream], 32 - HEADER_BITS)[0, 0]

    def decode_unit(self, msg, header, u, position_ref, emit):
        words = header >> 16
        reference = header & 0xFFFF
        reference = jnp.full((64, 128), reference | (reference << 16), jnp.int32)

        @pl.when(u == 0)
        def _():
            position_ref[...] = _in_first_lane(HEADER_BITS)
            msg[pl.ds(self.stream + words, self.guard)] = jnp.zeros((self.guard, *WORD), jnp.int32)

        def rebuild(i, group, top_bits=None):
            at = UNIT_WORDS * u + BLOCK_WORDS * i
            signs = msg[at + 8]
            sign = jnp.concatenate([signs << j if j else signs for j in range(8)], axis=0) & _rep(0x80)
            low = msg[pl.ds(at, 8)].reshape(64, 128)
            index = _from_rank((group << 2) | (_shr(low, 6) & _rep(0x03)))
            high = (_shr(index, 2) & _rep(0x1F)) | sign
            if top_bits is not None:
                high = high | top_bits
            low = (low & _rep(0x3F)) | ((index << 6) & _rep(0xC0))
            pairs = jnp.concatenate([reference - half for half in _swap_bytes(low, high)], axis=1)
            emit(i, pltpu.bitcast(pairs, jnp.bfloat16).astype(jnp.float32))

        @pl.when(words == self.raw_words)
        def _():
            for i in range(2):
                got = [msg[self.stream + 1 + 7 * (2 * u + i) + j] for j in range(7)]
                last = _shr(got[0] & _rep(0x80), 1)
                for j in range(1, 7):
                    last = last | _shr(got[j] & _rep(0x80), j + 1)
                high = jnp.concatenate(got + [last], axis=0)
                rebuild(i, high & _rep(0x1F), high & _rep(0x60))

        @pl.when(words < self.raw_words)
        def _():
            position = position_ref[...]
            for i in range(2):
                base = self._base(2 * u + i, words)
                drift = _shr(position, 5) - base
                near = msg[pl.ds(self.stream + base, self.window + 3)]
                near = [near[k] for k in range(self.window + 3)]
                hop = pl.next_power_of_2(self.window) // 2
                while hop:
                    moved = (drift & hop) != 0
                    near = [jnp.where(moved, near[k + hop], near[k]) if k + hop < len(near) else near[k]
                            for k in range(hop + 3)]
                    hop //= 2
                bit = position & 31
                rest = 31 - bit
                chain = [(near[k] << bit) | _shr(_shr(near[k + 1], 1), rest) for k in range(3)]
                groups = []
                for j in range(8):
                    code = chain[0]
                    for k in range(4):
                        zeros = lax.clz(code)
                        if k < 3:
                            code = (code << 1) << zeros
                        length = zeros + 4 if k == 0 else length + zeros
                        group = zeros if k == 0 else group | (zeros << (8 * k))
                    groups.append(group)
                    position = position + length
                    right = 32 - length
                    chain = [
                        (chain[k] << length) | _shr(chain[k + 1], right) if k + 1 < len(chain)
                        else chain[k] << length
                        for k in range(min(3, 7 - j))
                    ]
                rebuild(i, jnp.concatenate(groups, axis=0))
            position_ref[...] = position


class _HostInts:
    minimum, maximum = min, max
    where = staticmethod(lambda condition, a, b: a if condition else b)


class _Schedule:
    ahead, lag = 3, 2
    group = 4
    slots = 2

    def __init__(self, units, chunks, stream_pieces, lead, closing_steps):
        self.units, self.chunks, self.stream_pieces, self.lead = units, chunks, stream_pieces, lead
        self.pieces = units + stream_pieces
        self.jobs = units + closing_steps
        self.total_pieces = chunks * self.pieces
        self.steps = self.total_pieces + self.ahead + self.lag
        self.first_load_step = self.ahead + lead + stream_pieces - 2
        self.drain_piece = self.pieces // 2
        self._check()

    def stream_index(self, c, k, xp=jnp):
        return k - xp.where(c == 0, self.lead, 0)

    def _decodable(self, c, k, xp):
        whole_stream = self.stream_index(c, k, xp) >= self.stream_pieces - 1
        n = c * self.units + xp.where(whole_stream, k - self.stream_pieces + 1, 0)
        return xp.where(c < 0, 0, xp.minimum(n, self.chunks * self.units))

    def plan(self, t, at_x, at_y, encoding, jobs, done_x, done_y, xp=jnp):
        spare = (encoding > at_x[0] + 1) | (encoding == self.chunks)
        end_x = xp.minimum(self._decodable(*at_x, xp), done_x + 1 + xp.where(spare, 1 - (t & 1), 0))
        end_y = xp.minimum(self._decodable(*at_y, xp), done_y + 1 + xp.where(spare, t & 1, 0))
        busy = end_x - done_x + end_y - done_y
        quota = xp.where((t == 0) | (busy > 1), 1, xp.where(busy == 1, 2, 4))
        limit = xp.minimum(xp.maximum(at_x[0], 0) + 2, self.chunks) * self.jobs
        return xp.minimum(jobs + quota, limit), end_x, end_y

    def gives_credit(self, piece):
        return ((piece & (self.group - 1)) == self.group - 1) & (piece + self.group + 1 < self.total_pieces)

    def takes_credit(self, piece):
        return ((piece & (self.group - 1)) == 0) & (piece >= 2 * self.group)

    def _check(self):
        assert max(self.ahead, self.lag) <= self.group and self.chunks >= self.slots
        jobs = done_x = done_y = 0
        for t in range(self.steps):
            on_x, on_y = t - self.ahead, t - self.ahead - self.lag
            for piece, done in ((on_x, done_x), (on_y, done_y)):
                old = (piece + 2 * self.group) // self.pieces - self.slots
                if piece >= 0 and self.gives_credit(piece) and old >= 0:
                    assert done >= (old + 1) * self.units
                    assert piece > (old + 1) * self.pieces + self.drain_piece
            end, done_x, done_y = self.plan(
                t, divmod(on_x, self.pieces), divmod(on_y, self.pieces), jobs // self.jobs,
                jobs, done_x, done_y, _HostInts)
            for job in range(jobs, end):
                if job % self.jobs == 0:
                    assert t >= (job // self.jobs - self.slots + 1) * self.pieces
            assert end >= jobs and (done_x == 0 or t >= self.first_load_step)
            jobs = end
            if t < self.total_pieces:
                c, k = divmod(t, self.pieces)
                early = self.stream_index(c, k, _HostInts) < 0
                assert jobs >= (k + 1 if early else (c + 1) * self.jobs)
        assert done_x == done_y == self.chunks * self.units and jobs == self.chunks * self.jobs


def _reduce_scatter(x, *, units, stream_pieces, lead, closing_steps, window, back, tile_stride,
                    vmem_mib):
    _, m, n = x.shape
    assert n == 2 * COLS and m % (UNIT_ROWS * tile_stride) == 0 and m % (2 * UNIT_ROWS * units) == 0
    half_units = m // (2 * UNIT_ROWS)
    slabs = m // (UNIT_ROWS * tile_stride)
    codec = _Codec(units, window, back, closing_steps)
    plan = _Schedule(units, half_units // units, stream_pieces, lead, closing_steps)
    slots, group = plan.slots, plan.group
    assert codec.min_words >= UNIT_WORDS + stream_pieces
    send_depth, own_depth = 8, 2

    def body(x_ref, out_ref, stage_send, stage_x, stage_y, outbox, inbox_x, inbox_y, positions, lengths,
             headers_x, headers_y, stage_send_sem, stage_x_sem, stage_y_sem, sent_sem, forwarded_sem,
             recv_x_sem, recv_y_sem, credit_x_sem, credit_y_sem, *codec_scratch):
        mx, my = lax.axis_index("x"), lax.axis_index("y")
        peer_x, peer_y = (1 - mx, my), (mx, 1 - my)
        own_cols = pl.ds(pl.multiple_of(mx * COLS, COLS), COLS)
        peer_cols = pl.ds(pl.multiple_of((1 - mx) * COLS, COLS), COLS)
        first_x, first_y = my * half_units, (1 - my) * half_units

        def place(unit):
            return unit >> _log2(tile_stride), unit & (tile_stride - 1)

        def loader(first, cols, stage, sem):
            def load(g):
                s, k = place(first + g)
                slot = g & (stage.shape[0] - 1)
                src = x_ref.at[pl.ds(16 * s, 16), pl.ds(pl.multiple_of(8 * k, 8), 8), cols]
                return pltpu.make_async_copy(src, stage.at[slot], sem.at[slot])
            return load

        load_send = loader(first_x, peer_cols, stage_send, stage_send_sem)
        load_x = loader(first_x, own_cols, stage_x, stage_x_sem)
        load_y = loader(first_y, own_cols, stage_y, stage_y_sem)

        def piece(src, dst, send_sem, recv_sem, peer, c, k, words):
            q = plan.stream_index(c, k)
            share = ((words - UNIT_WORDS) * ((1 << 16) // (stream_pieces - 1))) >> 8
            begin = jnp.where(q == 0, 0, UNIT_WORDS + (((q - 1) * share) >> 8))
            end = jnp.where(q == stream_pieces - 1, words, UNIT_WORDS + ((q * share) >> 8))
            in_stream = (q >= 0) & (q < stream_pieces)
            unit = jnp.where(q < 0, k, k - stream_pieces)
            span = pl.ds(jnp.where(in_stream, codec.stream + begin, UNIT_WORDS * unit),
                         jnp.where(in_stream, end - begin, UNIT_WORDS))
            slot = c & (slots - 1)
            return pltpu.make_async_remote_copy(
                src.at[slot, span], dst.at[slot, span], send_sem.at[slot],
                recv_sem.at[(c * plan.pieces + k) & (2 * group - 1)],
                device_id=peer, device_id_type=MESH)

        def wait_all_sent(box, sem, slot, words):
            message = box.at[slot, pl.ds(0, codec.stream + words)]
            pltpu.make_async_copy(message, message, sem.at[slot]).wait()

        def take_credit(sem, index):
            @pl.when(plan.takes_credit(index))
            def _():
                pl.semaphore_wait(sem.at[(index >> _log2(group)) & 1], 1)

        def give_credit(sem, index, peer):
            @pl.when(plan.gives_credit(index))
            def _():
                pl.semaphore_signal(
                    sem.at[(index >> _log2(group)) & 1], 1, device_id=peer, device_id_type=MESH)

        def encoder_job(_, at):
            c, job = at
            slot = c & (slots - 1)

            @pl.when(job < units)
            def _():
                g = c * units + job
                src = stage_send.at[g & (send_depth - 1)]
                load_send(g).wait()

                @pl.when(job == 0)
                def _():
                    codec.open(src, codec_scratch)

                    @pl.when(c >= slots)
                    def _():
                        wait_all_sent(outbox, sent_sem, slot, lengths[slot])

                codec.encode_unit(src, job, outbox.at[slot], codec_scratch)

                @pl.when(g + send_depth < half_units)
                def _():
                    load_send(g + send_depth).start()

            @pl.when(job >= units)
            def _():
                codec.close(job - units, outbox.at[slot], codec_scratch, lengths, slot)

            return advance(at, plan.jobs)

        def receive(inbox, sem, headers, c, k):
            slot = c & (slots - 1)
            piece(inbox, inbox, forwarded_sem, sem, peer_y, c, k, headers[slot] >> 16).wait_recv()

            @pl.when(plan.stream_index(c, k) == 0)
            def _():
                headers[slot] = codec.header(inbox.at[slot])

        def add_unit(g, inbox, headers, load, stage, first, position_ref):
            slot = (g >> _log2(units)) & (slots - 1)
            s, k = place(first + g)
            load(g).wait()

            def emit(i, remote):
                own = stage[g & (own_depth - 1), :, :, 256 * i:256 * (i + 1)].reshape(UNIT_ROWS, 256)
                rows = pl.ds(pl.multiple_of(k * COLS + 256 * i, 256), 256)
                out_ref[s, rows, :] = (own + remote).T.astype(jnp.bfloat16)

            codec.decode_unit(inbox.at[slot], headers[slot], g & (units - 1), position_ref, emit)

            @pl.when(g + own_depth < half_units)
            def _():
                load(g + own_depth).start()

        def advance(at, period):
            wraps = at[1] == period - 1
            return jnp.where(wraps, at[0] + 1, at[0]), jnp.where(wraps, 0, at[1] + 1)

        def step(t, carry):
            at_send, at_x, at_y, at_encoder, done_x, done_y = carry

            @pl.when((at_x[0] >= 0) & (at_x[0] < plan.chunks))
            def _():
                c, k = at_x
                receive(inbox_x, recv_x_sem, headers_x, c, k)
                take_credit(credit_y_sem, t - plan.ahead)
                piece(inbox_x, inbox_y, forwarded_sem, recv_y_sem, peer_y, c, k,
                      headers_x[c & (slots - 1)] >> 16).start()
                give_credit(credit_x_sem, t - plan.ahead, peer_x)

                @pl.when((k == plan.drain_piece) & (c >= 1))
                def _():
                    slot = (c - 1) & (slots - 1)
                    wait_all_sent(inbox_x, forwarded_sem, slot, headers_x[slot] >> 16)

            jobs = at_encoder[0] * plan.jobs + at_encoder[1]
            end_jobs, end_x, end_y = plan.plan(t, at_x, at_y, at_encoder[0], jobs, done_x, done_y)
            at_encoder = lax.fori_loop(jobs, end_jobs, encoder_job, at_encoder)

            @pl.when(t == 0)
            def _():
                pl.semaphore_wait(barrier, 2)

            @pl.when(at_send[0] < plan.chunks)
            def _():
                c, k = at_send
                take_credit(credit_x_sem, t)
                piece(outbox, inbox_x, sent_sem, recv_x_sem, peer_x, c, k, lengths[c & (slots - 1)]).start()

            @pl.when(t == plan.first_load_step)
            def _():
                for g in range(own_depth):
                    load_x(jnp.int32(g)).start()
                    load_y(jnp.int32(g)).start()

            @pl.loop(done_x, end_x)
            def _(g):
                add_unit(g, inbox_x, headers_x, load_x, stage_x, first_x, positions.at[0])

            @pl.when(at_y[0] >= 0)
            def _():
                receive(inbox_y, recv_y_sem, headers_y, *at_y)
                give_credit(credit_y_sem, t - plan.ahead - plan.lag, peer_y)

            @pl.loop(done_y, end_y)
            def _(g):
                add_unit(g, inbox_y, headers_y, load_y, stage_y, first_y, positions.at[1])

            return (*(advance(at, plan.pieces) for at in (at_send, at_x, at_y)), at_encoder, end_x, end_y)

        barrier = pltpu.get_barrier_semaphore()
        for peer in (peer_x, peer_y):
            pl.semaphore_signal(barrier, 1, device_id=peer, device_id_type=MESH)
        for g in range(send_depth):
            load_send(jnp.int32(g)).start()
        for slot in range(slots):
            lengths[slot] = jnp.int32(codec.min_words)
            headers_x[slot] = jnp.int32(codec.min_words << 16)
            headers_y[slot] = jnp.int32(codec.min_words << 16)

        start = [(0, 0), divmod(-plan.ahead, plan.pieces), divmod(-plan.ahead - plan.lag, plan.pieces), (0, 0)]
        start = tuple((jnp.int32(c), jnp.int32(k)) for c, k in start)
        lax.fori_loop(0, plan.steps, step, (*start, jnp.int32(0), jnp.int32(0)))

        for slot in range(slots):
            wait_all_sent(outbox, sent_sem, slot, lengths[slot])
        slot = (plan.chunks - 1) % slots
        wait_all_sent(inbox_x, forwarded_sem, slot, headers_x[slot] >> 16)

    dma, regular = pltpu.SemaphoreType.DMA, pltpu.SemaphoreType.REGULAR
    box = pltpu.VMEM((slots, codec.message_words, *WORD), jnp.int32)
    per_slot = pltpu.SMEM((slots,), jnp.int32)
    out = pl.pallas_call(
        body,
        out_shape=pltpu.VMEM((slabs, tile_stride * COLS, UNIT_ROWS), jnp.bfloat16),
        in_specs=[pl.BlockSpec(memory_space=pl.ANY)],
        out_specs=pl.BlockSpec(memory_space=pltpu.VMEM),
        scratch_shapes=[
            *(pltpu.VMEM((depth, 16, 8, COLS), jnp.float32) for depth in (send_depth, own_depth, own_depth)),
            box, box, box,
            pltpu.VMEM((2, *WORD), jnp.int32),
            per_slot, per_slot, per_slot,
            dma((send_depth,)), dma((own_depth,)), dma((own_depth,)), dma((slots,)), dma((slots,)),
            dma((2 * group,)), dma((2 * group,)), regular((2,)), regular((2,)),
            *codec.scratch_shapes(),
        ],
        compiler_params=pltpu.CompilerParams(collective_id=0, vmem_limit_bytes=vmem_mib * 2**20),
    )(x.reshape(16 * slabs, 8 * tile_stride, n))
    out = out.transpose(0, 2, 1).reshape(slabs, 16, 8, tile_stride, COLS)
    return out.transpose(0, 1, 3, 2, 4).reshape(m, COLS)


def pallas_dist_rs_xy_x_m65536_n1024_kernel(
    x: jax.Array,
):
    return _reduce_scatter(
        x, units=64, stream_pieces=12, lead=20, closing_steps=16, window=28, back=20,
        tile_stride=128, vmem_mib=60)
```
